```python
import numpy as np

kernel_name = "dist_mean_ax1_xy_m1024_n512"

def setup_inputs():
    return {"x": np.random.randn(2048, 1024).astype(np.float32)}

def reference(x: np.ndarray) -> np.ndarray:
    return np.mean(x, axis=1, keepdims=True)
```

```python
import jax
import jax.numpy as jnp
from jax import lax
from jax.experimental import pallas as pl
from jax.experimental.pallas import tpu as pltpu

_LANES = 128
_SUB = 8
_K = 32
_TAIL = (64, 56, 8)


def pallas_dist_mean_ax1_xy_m1024_n512_kernel(
    x: jax.Array,
):
    m, n = x.shape
    nb = m // _LANES
    n_global = n * 2
    assert m % _LANES == 0 and n % _LANES == 0 and sum(_TAIL) == _LANES

    bounds = [_K] + [b * _LANES for b in range(1, nb)]
    for t in _TAIL:
        bounds.append(bounds[-1] + t)
    chunks = list(zip(bounds[:-1], bounds[1:])) + [(0, _K)]
    n_head = nb - 1

    def body(x_ref, out_ref, buf, raw, part, recv, in_sems, send_sems, recv_sems):
        loads = [
            pltpu.make_async_copy(
                x_ref.at[pl.ds(lo, hi - lo)], buf.at[pl.ds(lo, hi - lo)], in_sems.at[c]
            )
            for c, (lo, hi) in enumerate(chunks)
        ]
        for cp in loads:
            cp.start()

        peer = (lax.axis_index("x"), 1 - lax.axis_index("y"))
        barrier = pltpu.get_barrier_semaphore()
        pl.semaphore_signal(
            barrier, inc=1, device_id=peer, device_id_type=pl.DeviceIdType.MESH
        )

        def rdma(k, src, dst):
            return pltpu.make_async_remote_copy(
                src_ref=src,
                dst_ref=dst,
                send_sem=send_sems.at[k],
                recv_sem=recv_sems.at[k],
                device_id=peer,
                device_id_type=pl.DeviceIdType.MESH,
            )

        send_raw = rdma(0, x_ref.at[pl.ds(0, _K)], raw)
        send_head = rdma(1, part.at[pl.ds(0, nb - 1)], recv.at[pl.ds(0, nb - 1)])
        send_last = rdma(2, part.at[pl.ds(nb - 1, 1)], recv.at[pl.ds(nb - 1, 1)])

        pl.semaphore_wait(barrier, 1)
        send_raw.start()

        lane = lax.broadcasted_iota(jnp.int32, (_SUB, _LANES), 1)
        sub = lax.broadcasted_iota(jnp.int32, (_SUB, _LANES), 0)
        diag = lane - sub
        zero = jnp.zeros((_SUB, _LANES), jnp.float32)

        def fold(ref, r):
            t = [ref[r : r + _SUB, j : j + _LANES] for j in range(0, n, _LANES)]
            while len(t) > 1:
                t = [a + b for a, b in zip(t[0::2], t[1::2])] + t[len(t) & ~1 :]
            return t[0]

        def place(acc, folded):
            for r, p in folded:
                s = jnp.sum(p, axis=1, keepdims=True)
                acc = jnp.where(diag == r % _LANES, s, acc)
            return acc

        def to_row(acc):
            return jnp.sum(acc, axis=0, keepdims=True)

        def folded_chunk(c):
            loads[c].wait()
            lo, hi = chunks[c]
            return [(r, fold(buf, r)) for r in range(lo, hi, _SUB)]

        for c in range(n_head):
            part[c] = to_row(place(zero, folded_chunk(c)))
        send_head.start()

        acc = place(zero, folded_chunk(n_head))
        pending = []
        for c in range(n_head + 1, n_head + len(_TAIL)):
            pending += folded_chunk(c)
        part[nb - 1] = to_row(place(acc, pending))
        send_last.start()

        mine_raw = folded_chunk(len(chunks) - 1)
        send_raw.wait_recv()
        both = to_row(place(zero, [(r, p + fold(raw, r)) for r, p in mine_raw]))

        scale = 1.0 / n_global
        send_head.wait_recv()
        out_ref[0] = (part[0] + recv[0] + both) * scale
        out_ref[1 : nb - 1] = (part[1 : nb - 1] + recv[1 : nb - 1]) * scale
        mine_last = part[nb - 1]
        send_raw.wait_send()
        send_head.wait_send()
        send_last.wait_send()
        send_last.wait_recv()
        out_ref[nb - 1] = (mine_last + recv[nb - 1]) * scale

    params = dict(collective_id=0)
    if hasattr(pltpu.CompilerParams, "disable_semaphore_checks"):
        params["disable_semaphore_checks"] = True

    out = pl.pallas_call(
        body,
        out_shape=jax.ShapeDtypeStruct((nb, 1, _LANES), jnp.float32),
        in_specs=[pl.BlockSpec(memory_space=pl.ANY)],
        out_specs=pl.BlockSpec(memory_space=pltpu.VMEM),
        scratch_shapes=[
            pltpu.VMEM((m, n), jnp.float32),
            pltpu.VMEM((_K, n), jnp.float32),
            pltpu.VMEM((nb, 1, _LANES), jnp.float32),
            pltpu.VMEM((nb, 1, _LANES), jnp.float32),
            pltpu.SemaphoreType.DMA((len(chunks),)),
            pltpu.SemaphoreType.DMA((3,)),
            pltpu.SemaphoreType.DMA((3,)),
        ],
        compiler_params=pltpu.CompilerParams(**params),
    )(x)
    return out.reshape(m, 1)
```
